```python
import numpy as np

kernel_name = "dist_sparse_attn_strided_kvseq_b1_sq256_skv4096_hq8_dh128"

def setup_inputs():
    x = np.random.randn(1, 256, 1024).astype(np.float32)
    Wq = np.random.randn(1024, 1024).astype(np.float32) * 0.02
    K_ext = np.random.randn(1, 16384, 8, 128).astype(np.float32)
    V_ext = np.random.randn(1, 16384, 8, 128).astype(np.float32)
    Wo = np.random.randn(1024, 1024).astype(np.float32) * 0.02
    return {"x": x, "Wq": Wq, "K_ext": K_ext, "V_ext": V_ext, "Wo": Wo}

def reference(x, Wq, K_ext, V_ext, Wo):
    B, Sq, Skv, Hq, Dh = 1, 256, 16384, 8, 128
    Q = (x @ Wq).reshape(B, Sq, Hq, Dh)
    qb = (np.arange(Sq) // 64)[:, None]
    kb = (np.arange(Skv) // 64)[None, :]
    mask = (qb == kb) | ((kb % 4) == (qb % 4))
    scores = np.einsum('bihd,bjhd->bhij', Q, K_ext).astype(np.float32) * 0.08838834764831843
    scores = np.where(mask[None, None, :, :], scores, -1e9)
    scores_max = scores.max(axis=-1, keepdims=True)
    w = np.exp(scores - scores_max)
    row_keep = mask.any(axis=1)
    w_sum = np.where(row_keep[None, None, :, None], w.sum(axis=-1, keepdims=True), 1.0)
    w = w / w_sum
    w = np.where(row_keep[None, None, :, None], w, 0.0)
    ctx = np.einsum('bhij,bjhd->bihd', w, V_ext).reshape(B, Sq, Hq * Dh)
    return ctx @ Wo
```

```python
import jax
import jax.numpy as jnp
from jax import lax
from jax.experimental import pallas as pl
from jax.experimental.pallas import tpu as pltpu

N_DEV = 4
SQ = 256
D_MODEL = 1024
HQ = 8
DH = 128
BLK = 64
N_QB = SQ // BLK
N_KB = 16
KEYS = N_KB * BLK
GRP = 4
N_EARLY = N_QB * GRP
N_UNITS = N_QB * HQ
LAST = N_UNITS - 1
N_RS = 6
WINDOW = 10
MERGE_ITERS = (8, 11, 14, 17, 21, 25)
PROJ_ITERS = (12, 14, 17, 20)
A2A_ITERS = {29: 24, 30: 25}
V_SPLIT = 4
HALF = D_MODEL // 2
LATE_Q_AT = 3
IDLE = 2
OFF_ITERS = tuple(range(0, 26))
PRE = ('q', 'q', 'x')
PRE_AT = (0, 0, 1, 1, 2, 3)
DIRS = ('+', '-')
OFF_END = 31
OFF_NB = 1
NARROW = 1
OCOLS = 384
WOL = ((0, 512), (512, 1024))
WOL7 = ((0, 512), (512, 1024))
FOLD_AT = 24
MERGE_AT = {0: [26], 1: [27], 2: [28], 3: [29], 5: [30]}
WEIGHTS_AT = 6
SCALE_LOG2 = 0.08838834764831843 * 1.4426950408889634

BULK_ORDER = (1, 3, 2)
FAST_ORDER = (2, 1, 3)

MESH = pl.DeviceIdType.MESH


def _col_to_row(col):
    r = lax.broadcasted_iota(jnp.int32, (BLK, DH), 0)
    c = lax.broadcasted_iota(jnp.int32, (BLK, DH), 1)
    return jnp.sum(jnp.where(r == c, col, 0.0), axis=0, keepdims=True)


def _row_to_col(row):
    r = lax.broadcasted_iota(jnp.int32, (BLK, DH), 0)
    c = lax.broadcasted_iota(jnp.int32, (BLK, DH), 1)
    return jnp.sum(jnp.where(r == c, row, 0.0), axis=1, keepdims=True)


def _chip_weights(lses):
    m = jnp.maximum(jnp.maximum(lses[0], lses[1]), jnp.maximum(lses[2], lses[3]))
    es = [jnp.exp2(t - m) for t in lses]
    inv = 1.0 / (es[0] + es[1] + es[2] + es[3])
    return [e * inv for e in es]


def _body(x_hbm, wq_hbm, k_hbm, v_hbm, wo_hbm, out_ref,
          kbuf, vbuf, xbuf, xh, wqbuf, wqbf, qpart, qsend, qrecv, wobuf, wobf, wolbuf, wo7bf,
          q_all, o_all, lse_all, ctx_all, osl, wcol,
          ksem, vsem, vlsem, insem, wolsem,
          send, x_recv, p_recv, q_recv, o_recv, l_recv, c_recv, s_recv):
    me = lax.axis_index("i")
    owner = me != IDLE
    owners = [c for c in range(N_DEV) if c != IDLE]
    widths = [OCOLS - DH if c == NARROW else OCOLS for c in owners]
    starts = [sum(widths[:i]) for i in range(3)]
    col0 = pl.multiple_of(
        jnp.where(me == owners[0], starts[0],
                  jnp.where(me == owners[1], starts[1], starts[2])), DH)
    odd = lax.rem(me, 2) == 1
    first = jnp.where(odd, N_DEV - me, 2)
    second = jnp.where(odd, 2, 1)
    tail_order = (first, second, 6 - first - second)
    x_send, q_send, o_send, l_send, c_send, s_send = (send.at[i] for i in range(6))
    off_send = send.at[6]
    p_send = send.at[7]
    ka = me // 2
    cb = lax.rem((me + 1) // 2, 2)
    d_x = jnp.where(odd, 3, 1)
    d_q = jnp.where(odd, 1, 3)
    OFF_PRE = 2 * len(PRE)
    off_n = (OFF_PRE + len(OFF_ITERS)) // 2
    off0 = OFF_END - off_n

    def lookup(u, table):
        r = jnp.int32(-1)
        for at, val in table:
            r = jnp.where(u == at, val, r)
        return r

    pieces = [(j, c0, c1) for j in range(GRP)
              for (c0, c1) in (WOL7 if j == GRP - 1 else WOL)]

    def peer(d):
        return lax.rem(me + d, N_DEV)

    def source(d):
        return lax.rem(me + (N_DEV - d), N_DEV)

    def unit_coords(u):
        hi, lo = u // GRP, lax.rem(u, GRP)
        early = u < N_EARLY
        return jnp.where(early, hi, lo), jnp.where(early, lo, hi)

    def head_of(slot):
        idx = lax.rem(slot, GRP)
        return (idx // 2) * GRP + (slot // GRP) * 2 + lax.rem(idx, 2)

    def unit_kv(u):
        qb, slot = unit_coords(u)
        return qb, head_of(slot)

    def k_copy(u):
        qb, h = unit_kv(u)
        return pltpu.make_async_copy(k_hbm.at[:, qb, :, h, :], kbuf.at[u], ksem.at[u])

    def v_copy(u):
        qb, h = unit_kv(u)
        return pltpu.make_async_copy(v_hbm.at[:, qb, :, h, :], vbuf.at[u], vsem.at[u])

    def kv_rest_copies(u):
        qb, h = unit_kv(u)
        rest = pl.ds(OFF_NB, N_KB - OFF_NB)
        return [pltpu.make_async_copy(src.at[rest, qb, :, h, :], dst.at[u, rest], sem.at[u])
                for src, dst, sem in ((k_hbm, kbuf, ksem), (v_hbm, vbuf, vsem))]

    def swap_copy(u, d, src, dst, sem):
        qb, h = unit_kv(u)
        part = pl.ds(0, OFF_NB)
        return pltpu.make_async_remote_copy(
            src_ref=src.at[part, qb, :, h, :], dst_ref=dst.at[u, part],
            send_sem=off_send, recv_sem=sem.at[u],
            device_id=(peer(d),), device_id_type=MESH)

    dir_of = {'x': d_x, 'q': d_q, '+': 1, '-': 3}

    def pre_swaps(point):
        for j in range(OFF_PRE):
            if PRE_AT[j] == point:
                swap_copy(off0 + j // 2, dir_of[PRE[j // 2]],
                          *((k_hbm, kbuf, ksem), (v_hbm, vbuf, vsem))[j % 2]).start()

    def v_last_copy(j):
        n = N_KB // V_SPLIT
        return pltpu.make_async_copy(
            v_hbm.at[pl.ds(j * n, n), N_QB - 1, :, HQ - 1, :],
            vbuf.at[LAST, pl.ds(j * n, n)], vlsem.at[j])

    def wol_copy(i):
        j, c0, c1 = pieces[i]
        return pltpu.make_async_copy(
            wo_hbm.at[j // 2, 1, pl.ds((j % 2) * DH, DH), pl.ds(c0, c1 - c0)],
            wolbuf.at[j, :, pl.ds(c0, c1 - c0)], wolsem.at[i])

    def remote(ref, send_sem, recv_sem, d):
        return pltpu.make_async_remote_copy(
            src_ref=ref, dst_ref=ref, send_sem=send_sem, recv_sem=recv_sem,
            device_id=(peer(d),), device_id_type=MESH)

    def wait_bytes(ref, sem):
        pltpu.make_async_copy(ref, ref, sem).wait()

    x_copy = pltpu.make_async_copy(
        x_hbm.at[0, pl.ds(pl.multiple_of(cb * (SQ // 2), SQ // 2), SQ // 2),
                 pl.ds(pl.multiple_of(ka * HALF, HALF), HALF)], xbuf, insem.at[0])
    wq_copy = pltpu.make_async_copy(
        wq_hbm.at[pl.ds(pl.multiple_of(ka * HALF, HALF), HALF),
                  pl.ds(pl.multiple_of(cb * HALF, HALF), HALF)], wqbuf, insem.at[1])
    wide = jnp.logical_and(owner, me != NARROW)

    def by_width(chip, fn):
        @pl.when(jnp.logical_and(chip != IDLE, chip != NARROW))
        def _():
            fn(OCOLS)

        @pl.when(chip == NARROW)
        def _():
            fn(OCOLS - DH)

    def wo_copy(w):
        return pltpu.make_async_copy(
            wo_hbm.at[:, 0, :, pl.ds(col0, w)],
            wobuf.at[:, :, pl.ds(0, w)], insem.at[2])

    x_copy.start()
    barrier = pltpu.get_barrier_semaphore()
    for d in FAST_ORDER:
        pl.semaphore_signal(barrier, inc=1, device_id=(peer(d),), device_id_type=MESH)
    wq_copy.start()

    by_width(me, lambda w: wo_copy(w).start())

    for u in range(WINDOW):
        k_copy(u).start()
        v_copy(u).start()

    x_copy.wait()
    xh[cb] = xbuf[...].astype(jnp.bfloat16)
    pl.semaphore_wait(barrier, N_DEV - 1)
    remote(xh.at[cb], x_send, x_recv, d_x).start()
    pre_swaps(0)
    wq_copy.wait()
    wqbf[...] = wqbuf[...].astype(jnp.bfloat16)

    def load_wo(w):
        wo_copy(w).wait()
        wobf[:, :w] = wobuf[:, :, :w].reshape(GRP * DH, w).astype(jnp.bfloat16)

    by_width(me, load_wo)

    pre_swaps(1)
    wait_bytes(xh.at[1 - cb], x_recv)
    pre_swaps(2)
    q = jnp.dot(xh[...].reshape(SQ, HALF), wqbf[...],
                preferred_element_type=jnp.float32) * SCALE_LOG2
    for j in range(GRP):
        qj = q[:, j * DH:(j + 1) * DH].reshape(N_QB, BLK, DH)
        qpart[j] = qj
        qsend[j] = qj.astype(jnp.bfloat16)

    q_parts = ((0, 0, 1), (0, 1, N_QB - 1), (1, 0, N_QB))

    def p_slice(ref, kind):
        late, q0, nq = q_parts[kind]
        return ref.at[pl.ds(2 * late, 2), pl.ds(q0, nq)]

    def q_slice(kind, half):
        late, q0, nq = q_parts[kind]
        return q_all.at[pl.ds(late * GRP + 2 * half, 2), pl.ds(q0, nq)]

    for kind in range(3):
        pltpu.make_async_remote_copy(
            src_ref=p_slice(qsend, kind), dst_ref=p_slice(qrecv, kind), send_sem=p_send,
            recv_sem=p_recv.at[kind], device_id=(peer(d_q),), device_id_type=MESH).start()

    def finish_q(kind):
        wait_bytes(p_slice(qrecv, kind), p_recv.at[kind])
        q_slice(kind, cb)[...] = (
            p_slice(qpart, kind)[...] + p_slice(qrecv, kind)[...].astype(jnp.float32)
        ).astype(jnp.bfloat16)
        remote(q_slice(kind, cb), q_send, q_recv.at[kind], d_x).start()

    pre_swaps(3)
    finish_q(0)
    pre_swaps(4)
    finish_q(1)

    def wait_q(kind):
        wait_bytes(q_slice(kind, 1 - cb), q_recv.at[kind])

    def wait_lse(u):
        for d in (1, 2, 3):
            wait_bytes(lse_all.at[source(d), u], l_recv.at[u * 3 + d - 1])

    def wait_o(u):
        for d in (1, 2, 3):
            wait_bytes(o_all.at[source(d), u], o_recv.at[u * 3 + d - 1])

    def wait_ctx(g):
        for d in (1, 2, 3):
            wait_bytes(ctx_all.at[g * GRP + source(d)], c_recv.at[g * 3 + d - 1])

    def merge_wait(units):
        for u in units:
            wait_lse(u)
            wait_o(u)

    def merge(units):
        for u in units:
            ws = _chip_weights([lse_all[c, u] for c in range(N_DEV)])
            acc = None
            for c in range(N_DEV):
                term = _row_to_col(ws[c]) * o_all[c, u].astype(jnp.float32)
                acc = term if acc is None else acc + term
            ctx_all[u] = acc.astype(jnp.bfloat16)

    def send_lse(u, d):
        remote(lse_all.at[me, u], l_send, l_recv.at[u * 3 + d - 1], d).start()

    def send_o(u, d):
        remote(o_all.at[me, u], o_send, o_recv.at[u * 3 + d - 1], d).start()

    def scores(u, qb, h):
        k = kbuf[u].reshape(KEYS, DH).astype(jnp.bfloat16)
        s = lax.dot_general(q_all[h, qb], k, (((1,), (1,)), ((), ())),
                            preferred_element_type=jnp.float32)
        m = jnp.max(s, axis=1, keepdims=True)
        p = jnp.exp2(s - m)
        l = jnp.sum(p, axis=1, keepdims=True)
        lse_all[me, u] = _col_to_row(m + jnp.log2(l))
        return p.astype(jnp.bfloat16), 1.0 / l

    def unit_step(u, carry):
        qb, h = unit_coords(u)
        row = lax.rem(u, GRP)

        nxt = u + WINDOW
        swapped = jnp.logical_and(nxt >= off0, nxt < OFF_END)

        @pl.when(jnp.logical_and(nxt < LAST, jnp.logical_not(swapped)))
        def _():
            k_copy(nxt).start()
            v_copy(nxt).start()

        @pl.when(swapped)
        def _():
            for c in kv_rest_copies(nxt):
                c.start()

        chunk = lookup(u, [(at, OFF_PRE + j) for j, at in enumerate(OFF_ITERS)])
        fire = chunk >= 0
        for which, (src, dst, sem) in enumerate(((k_hbm, kbuf, ksem), (v_hbm, vbuf, vsem))):
            @pl.when(jnp.logical_and(fire, lax.rem(chunk, 2) == which))
            def _():
                uu = off0 + chunk // 2
                d = jnp.where(lax.rem(uu, 2) == 0, dir_of[DIRS[0]], dir_of[DIRS[1]])
                swap_copy(uu, d, src, dst, sem).start()

        @pl.when(u + WINDOW == LAST)
        def _():
            k_copy(LAST).start()
            for j in range(V_SPLIT):
                v_last_copy(j).start()

        @pl.when(u + WINDOW == LAST + 4)
        def _():
            for i in range(len(pieces)):
                wol_copy(i).start()

        for kind, at in enumerate((0, GRP, N_EARLY)):
            @pl.when(u == at)
            def _():
                wait_q(kind)

        @pl.when(u == LATE_Q_AT)
        def _():
            finish_q(2)

        k_copy(u).wait()
        v_copy(u).wait()
        p, inv_l = scores(u, qb, h)
        v = vbuf[u].reshape(KEYS, DH).astype(jnp.bfloat16)
        acc = jnp.dot(p, v, preferred_element_type=jnp.float32)
        o_all[me, u] = (acc * inv_l).astype(jnp.bfloat16)

        @pl.when(jnp.logical_and(u < N_RS * GRP, row != me))
        def _():
            d = lax.rem(row - me + N_DEV, N_DEV)
            send_lse(u, d)
            send_o(u, d)

        @pl.when(u >= N_RS * GRP)
        def _():
            for d in tail_order:
                send_lse(u, d)
                send_o(u, d)

        g1 = lookup(u, [(at, g) for g, at in enumerate(MERGE_ITERS)])
        mu = jnp.where(g1 >= 0, g1 * GRP + me, lookup(u, list(A2A_ITERS.items())))

        @pl.when(mu >= 0)
        def _():
            merge_wait([mu])
            merge([mu])

        @pl.when(g1 >= 0)
        def _():
            for d in BULK_ORDER:
                @pl.when(jnp.logical_or(g1 >= N_QB, peer(d) != IDLE))
                def _():
                    remote(ctx_all.at[mu], c_send, c_recv.at[g1 * 3 + d - 1], d).start()

        g = lookup(u, [(at, g) for g, at in enumerate(PROJ_ITERS)])

        @pl.when(jnp.logical_and(g >= 0, owner))
        def _():
            wait_ctx(g)

            def project_early(w):
                ctx = jnp.concatenate([ctx_all[g * GRP + i] for i in range(GRP)], axis=1)
                osl[me, g, :, :w] = jnp.dot(
                    ctx, wobf[:, :w], preferred_element_type=jnp.float32).astype(jnp.bfloat16)
                for d in BULK_ORDER:
                    remote(osl.at[me, g, :, pl.ds(0, w)], s_send, s_recv.at[d - 1], d).start()

            by_width(me, project_early)

        @pl.when(u == FOLD_AT)
        def _():
            for d in (1, 2, 3):
                by_width(source(d), lambda w: wait_bytes(
                    osl.at[source(d), :, :, pl.ds(0, w)], s_recv.at[d - 1]))
            for c, c0, w in zip(owners, starts, widths):
                out_ref[0, :, c0:c0 + w] = osl[c, :, :, :w].reshape(SQ, w).astype(jnp.float32)

        return carry

    lax.fori_loop(0, LAST, unit_step, 0)

    k_copy(LAST).wait()
    p, inv_l = scores(LAST, N_QB - 1, HQ - 1)
    for d in tail_order:
        send_lse(LAST, d)
    acc = None
    n = KEYS // V_SPLIT
    for j in range(V_SPLIT):
        v_last_copy(j).wait()
        v = vbuf[LAST, pl.ds(j * N_KB // V_SPLIT, N_KB // V_SPLIT)].reshape(n, DH)
        t = jnp.dot(p[:, j * n:(j + 1) * n], v.astype(jnp.bfloat16),
                    preferred_element_type=jnp.float32)
        acc = t if acc is None else acc + t
    o_all[me, LAST] = (acc * inv_l).astype(jnp.bfloat16)
    for d in tail_order:
        send_o(LAST, d)

    head = (N_QB - 1) * BLK

    def project(i):
        j, c0, c1 = pieces[i]
        wo = wolbuf[j, :, c0:c1].astype(jnp.bfloat16)
        n_rows = SQ
        if j == GRP - 1:
            wo7bf[:, c0:c1] = wo
            n_rows = head
        ctx = ctx_all[pl.ds((GRP + j) * GRP, n_rows // BLK)].reshape(n_rows, DH)
        out_ref[0, :n_rows, c0:c1] = out_ref[0, :n_rows, c0:c1] + jnp.dot(
            ctx, wo, preferred_element_type=jnp.float32)

    for g in range(N_QB, N_RS):
        wait_ctx(g)
    wait_bytes(xh.at[0], x_send)
    wait_bytes(qsend, p_send)
    wait_bytes(qsend, q_send)
    wait_bytes(ctx_all.at[pl.ds(0, 3 * N_RS - N_QB)], c_send)

    @pl.when(jnp.logical_not(owner))
    def _():
        wait_bytes(ctx_all.at[pl.ds(0, N_QB)], c_send)

    if off_n:
        wait_bytes(kbuf.at[pl.ds(0, 2 * off_n), pl.ds(0, OFF_NB)], off_send)

    by_width(me, lambda w: wait_bytes(osl.at[pl.ds(0, 3), :, :, pl.ds(0, w)], s_send))

    n_sent = (N_RS + N_UNITS - N_RS * GRP) * 3
    for i in range(len(pieces)):
        units = MERGE_AT.get(i, [])
        if units:
            merge_wait(units)
        if i == WEIGHTS_AT:
            wait_lse(LAST)
            wait_bytes(o_all.at[pl.ds(0, 2), pl.ds(0, n_sent // 2)], o_send)
            wait_bytes(lse_all.at[pl.ds(0, 2), pl.ds(0, n_sent // 2)], l_send)
        wol_copy(i).wait()
        project(i)
        merge(units)
        if i == WEIGHTS_AT:
            ws = _chip_weights([lse_all[c, LAST] for c in range(N_DEV)])
            for c in range(N_DEV):
                wcol[c] = jnp.broadcast_to(_row_to_col(ws[c]), (BLK, DH))

    wait_o(LAST)
    acc = None
    for c in range(N_DEV):
        term = wcol[c] * o_all[c, LAST].astype(jnp.float32)
        acc = term if acc is None else acc + term
    out_ref[0, head:] = out_ref[0, head:] + jnp.dot(
        acc.astype(jnp.bfloat16), wo7bf[...], preferred_element_type=jnp.float32)


def pallas_dist_sparse_attn_strided_kvseq_b1_sq256_skv4096_hq8_dh128_kernel(x, Wq, K_ext, V_ext, Wo):
    k5 = K_ext.reshape(N_KB, N_QB, BLK, HQ, DH)
    v5 = V_ext.reshape(N_KB, N_QB, BLK, HQ, DH)
    f32, bf16 = jnp.float32, jnp.bfloat16
    dma = pltpu.SemaphoreType.DMA
    return pl.pallas_call(
        _body,
        out_shape=jax.ShapeDtypeStruct((1, SQ, D_MODEL), f32),
        in_specs=[pl.BlockSpec(memory_space=pl.ANY)] * 5,
        out_specs=pl.BlockSpec(memory_space=pltpu.VMEM),
        scratch_shapes=[
            pltpu.VMEM((N_UNITS, N_KB, BLK, DH), f32),
            pltpu.VMEM((N_UNITS, N_KB, BLK, DH), f32),
            pltpu.VMEM((SQ // 2, HALF), f32),
            pltpu.VMEM((2, SQ // 2, HALF), bf16),
            pltpu.VMEM((HALF, HALF), f32),
            pltpu.VMEM((HALF, HALF), bf16),
            pltpu.VMEM((GRP, N_QB, BLK, DH), f32),
            pltpu.VMEM((GRP, N_QB, BLK, DH), bf16),
            pltpu.VMEM((GRP, N_QB, BLK, DH), bf16),
            pltpu.VMEM((2, 2 * DH, OCOLS), f32),
            pltpu.VMEM((GRP * DH, OCOLS), bf16),
            pltpu.VMEM((GRP, DH, D_MODEL), f32),
            pltpu.VMEM((DH, D_MODEL), bf16),
            pltpu.VMEM((HQ, N_QB, BLK, DH), bf16),
            pltpu.VMEM((N_DEV, N_UNITS, BLK, DH), bf16),
            pltpu.VMEM((N_DEV, N_UNITS, 1, DH), f32),
            pltpu.VMEM((N_UNITS, BLK, DH), bf16),
            pltpu.VMEM((N_DEV, N_QB, BLK, OCOLS), bf16),
            pltpu.VMEM((N_DEV, BLK, DH), f32),
            dma((N_UNITS,)), dma((N_UNITS,)), dma((V_SPLIT,)), dma((3,)),
            dma((3 * len(WOL) + len(WOL7),)),
            dma((8,)), dma, dma((3,)), dma((3,)),
            dma((3 * N_UNITS,)), dma((3 * N_UNITS,)),
            dma((3 * N_RS,)), dma((3,)),
        ],
        compiler_params=pltpu.CompilerParams(
            collective_id=0,
            vmem_limit_bytes=64 * 1024 * 1024,
            disable_semaphore_checks=True,
        ),
    )(x, Wq, k5, v5, Wo.reshape(2, 2, 2 * DH, D_MODEL))
```

```python
import jax
import jax.numpy as jnp
from jax import lax
from jax.experimental import pallas as pl
from jax.experimental.pallas import tpu as pltpu

N_DEV = 4
SQ = 256
D_MODEL = 1024
HALF = D_MODEL // 2
HQ = 8
DH = 128
BLK = 64
N_QB = SQ // BLK
N_KB = 16
KEYS = N_KB * BLK
GRP = 4
N_EARLY = N_QB * GRP
N_UNITS = N_QB * HQ
LAST = N_UNITS - 1
N_RS = 6
N_SLOTS = N_RS + N_UNITS - N_RS * GRP
WINDOW = 10

MERGE_ITERS = (9, 11, 14, 18, 22, 26)
PROJ_ITERS = (12, 15, 18, 21)
FWD_ITERS = (15, 18, 21, 24)
LATE_Q_AT = 3
FOLD_AT = 29

WIDE = 384
NARROW = 256
IDLE_CHIP = 2
NARROW_CHIP = 1
OWNER_COLS = ((0, 0, WIDE), (1, WIDE, NARROW), (3, WIDE + NARROW, WIDE))

PRE_SWAPS = (("q", 0, 0), ("q", 0, 1), ("q", 1, 1), ("x", 2, 2), ("x", 3, 3), ("x", 4, 4))
LOOP_SWAPS = 28
N_SWAPPED = len(PRE_SWAPS) + LOOP_SWAPS // 2
SWAP0 = LAST - N_SWAPPED

V_CUTS = (0, 12, 16)
PIECES = tuple((j, c) for j in range(GRP) for c in (0, HALF))
MERGE_AT = {0: (24, 25), 1: (26, 27), 2: (28,), 3: (29,), 5: (30,)}
WEIGHTS_AT = 6
Q_PARTS = ((0, 0, 1), (0, 1, N_QB - 1), (1, 0, N_QB))

SCALE_LOG2 = 0.08838834764831843 * 1.4426950408889634
MESH = pl.DeviceIdType.MESH
F32 = jnp.float32
BF16 = jnp.bfloat16


def _diagonal(val):
    r = lax.broadcasted_iota(jnp.int32, (BLK, DH), 0)
    c = lax.broadcasted_iota(jnp.int32, (BLK, DH), 1)
    return jnp.where(r == c, val, 0.0)


def _col_to_row(col):
    return jnp.sum(_diagonal(col), axis=0, keepdims=True)


def _row_to_col(row):
    return jnp.sum(_diagonal(row), axis=1, keepdims=True)


def _chip_weights(lses):
    m = jnp.maximum(jnp.maximum(lses[0], lses[1]), jnp.maximum(lses[2], lses[3]))
    es = [jnp.exp2(t - m) for t in lses]
    inv = 1.0 / (es[0] + es[1] + es[2] + es[3])
    return [e * inv for e in es]


def _lookup(u, iters):
    r = jnp.int32(-1)
    for g, at in enumerate(iters):
        r = jnp.where(u == at, g, r)
    return r


def _body(x_hbm, wq_hbm, k_hbm, v_hbm, wo_hbm, out_ref,
          kbuf, vbuf, xbuf, xh, wqbuf, wqbf, qpart, qsend, qrecv, wobuf, wobf, wolbuf,
          wo7bf, q_all, o_all, lse_all, ctx_all, osl, wcol,
          ksem, vsem, vlsem, insem, wolsem,
          send, x_recv, p_recv, q_recv, o_recv, l_recv, c_recv, sx_recv, s_recv):
    me = lax.axis_index("i")
    odd = lax.rem(me, 2) == 1
    owner = me != IDLE_CHIP
    k_half = me // 2
    c_half = lax.rem((me + 1) // 2, 2)
    d_x = jnp.where(odd, 3, 1)
    d_q = jnp.where(odd, 1, 3)
    first = jnp.where(odd, N_DEV - me, 2)
    second = jnp.where(odd, 2, 1)
    tail_order = (first, second, 6 - first - second)
    (x_send, p_send, q_send, o_send, l_send, c_send, s_send, f_send, w_send) = (
        send.at[i] for i in range(9))
    kv = ((k_hbm, kbuf, ksem), (v_hbm, vbuf, vsem))

    def peer(d):
        return lax.rem(me + d, N_DEV)

    def source(d):
        return lax.rem(me + (N_DEV - d), N_DEV)

    def unit_coords(u):
        hi, lo = u // GRP, lax.rem(u, GRP)
        early = u < N_EARLY
        return jnp.where(early, hi, lo), jnp.where(early, lo, hi)

    def unit_src(src, u, blocks):
        qb, slot = unit_coords(u)
        idx = lax.rem(slot, GRP)
        head = (idx // 2) * GRP + (slot // GRP) * 2 + lax.rem(idx, 2)
        return src.at[blocks, qb, :, head, :]

    def kv_copy(which, u, first_block=0):
        src, dst, sem = kv[which]
        blocks = pl.ds(first_block, N_KB - first_block)
        return pltpu.make_async_copy(unit_src(src, u, blocks), dst.at[u, blocks], sem.at[u])

    def swap_copy(which, u, d):
        src, dst, sem = kv[which]
        block = pl.ds(0, 1)
        return pltpu.make_async_remote_copy(
            src_ref=unit_src(src, u, block), dst_ref=dst.at[u, block],
            send_sem=w_send, recv_sem=sem.at[u],
            device_id=(peer(d),), device_id_type=MESH)

    def pre_swaps(point):
        for n, (link, *points) in enumerate(PRE_SWAPS):
            for which in range(2):
                if points[which] == point:
                    swap_copy(which, SWAP0 + n, d_q if link == "q" else d_x).start()

    def v_last_copy(j):
        blocks = pl.ds(V_CUTS[j], V_CUTS[j + 1] - V_CUTS[j])
        return pltpu.make_async_copy(
            v_hbm.at[blocks, N_QB - 1, :, HQ - 1, :], vbuf.at[LAST, blocks], vlsem.at[j])

    def late_wo_copy(i):
        j, c0 = PIECES[i]
        return pltpu.make_async_copy(
            wo_hbm.at[j // 2, 1, pl.ds((j % 2) * DH, DH), pl.ds(c0, HALF)],
            wolbuf.at[j, :, pl.ds(c0, HALF)], wolsem.at[i])

    def early_wo_copy(w):
        col0 = jnp.int32(0)
        for chip, start, _ in OWNER_COLS:
            col0 = jnp.where(me == chip, start, col0)
        return pltpu.make_async_copy(
            wo_hbm.at[:, 0, :, pl.ds(pl.multiple_of(col0, DH), w)],
            wobuf.at[:, :, pl.ds(0, w)], insem.at[2])

    def remote(ref, send_sem, recv_sem, d):
        return pltpu.make_async_remote_copy(
            src_ref=ref, dst_ref=ref, send_sem=send_sem, recv_sem=recv_sem,
            device_id=(peer(d),), device_id_type=MESH)

    def wait_bytes(ref, sem):
        pltpu.make_async_copy(ref, ref, sem).wait()

    def by_width(chip, fn):
        @pl.when(jnp.logical_and(chip != IDLE_CHIP, chip != NARROW_CHIP))
        def _():
            fn(WIDE)

        @pl.when(chip == NARROW_CHIP)
        def _():
            fn(NARROW)

    k_rows = pl.ds(pl.multiple_of(k_half * HALF, HALF), HALF)
    x_copy = pltpu.make_async_copy(
        x_hbm.at[0, pl.ds(pl.multiple_of(c_half * (SQ // 2), SQ // 2), SQ // 2), k_rows],
        xbuf, insem.at[0])
    wq_copy = pltpu.make_async_copy(
        wq_hbm.at[k_rows, pl.ds(pl.multiple_of(c_half * HALF, HALF), HALF)],
        wqbuf, insem.at[1])

    x_copy.start()
    barrier = pltpu.get_barrier_semaphore()
    for d in (2, 1, 3):
        pl.semaphore_signal(barrier, inc=1, device_id=(peer(d),), device_id_type=MESH)
    wq_copy.start()
    by_width(me, lambda w: early_wo_copy(w).start())
    for u in range(WINDOW):
        kv_copy(0, u).start()
        kv_copy(1, u).start()

    x_copy.wait()
    xh[c_half] = xbuf[...].astype(BF16)
    pl.semaphore_wait(barrier, N_DEV - 1)
    remote(xh.at[c_half], x_send, x_recv, d_x).start()
    pre_swaps(0)
    wq_copy.wait()
    wqbf[...] = wqbuf[...].astype(BF16)

    def load_early_wo(w):
        early_wo_copy(w).wait()
        wobf[:, :w] = wobuf[:, :, :w].reshape(GRP * DH, w).astype(BF16)

    by_width(me, load_early_wo)
    pre_swaps(1)
    wait_bytes(xh.at[1 - c_half], x_recv)
    pre_swaps(2)
    q = jnp.dot(xh[...].reshape(SQ, HALF), wqbf[...],
                preferred_element_type=F32) * SCALE_LOG2
    for j in range(GRP):
        qj = q[:, j * DH:(j + 1) * DH].reshape(N_QB, BLK, DH)
        qpart[j] = qj
        qsend[j] = qj.astype(BF16)

    def p_slice(ref, part):
        late, q0, nq = Q_PARTS[part]
        return ref.at[pl.ds(2 * late, 2), pl.ds(q0, nq)]

    def q_slice(part, half):
        late, q0, nq = Q_PARTS[part]
        return q_all.at[pl.ds(late * GRP + 2 * half, 2), pl.ds(q0, nq)]

    for part in range(len(Q_PARTS)):
        pltpu.make_async_remote_copy(
            src_ref=p_slice(qsend, part), dst_ref=p_slice(qrecv, part), send_sem=p_send,
            recv_sem=p_recv.at[part], device_id=(peer(d_q),), device_id_type=MESH).start()

    def finish_q(part):
        wait_bytes(p_slice(qrecv, part), p_recv.at[part])
        q_slice(part, c_half)[...] = (
            p_slice(qpart, part)[...] + p_slice(qrecv, part)[...].astype(F32)).astype(BF16)
        remote(q_slice(part, c_half), q_send, q_recv.at[part], d_x).start()

    pre_swaps(3)
    finish_q(0)
    pre_swaps(4)
    finish_q(1)

    def sem_index(slot, d):
        return slot * 3 + d - 1

    def all_slot(u):
        return u - N_RS * (GRP - 1)

    def send_lse(u, slot, d):
        remote(lse_all.at[me, u], l_send, l_recv.at[sem_index(slot, d)], d).start()

    def send_o(u, slot, d):
        remote(o_all.at[me, u], o_send, o_recv.at[sem_index(slot, d)], d).start()

    def wait_lse(u, slot):
        for d in (1, 2, 3):
            wait_bytes(lse_all.at[source(d), u], l_recv.at[sem_index(slot, d)])

    def wait_o(u, slot):
        for d in (1, 2, 3):
            wait_bytes(o_all.at[source(d), u], o_recv.at[sem_index(slot, d)])

    def wait_ctx(g):
        for d in (1, 2, 3):
            wait_bytes(ctx_all.at[g * GRP + source(d)], c_recv.at[sem_index(g, d)])

    def merge(u):
        ws = _chip_weights([lse_all[c, u] for c in range(N_DEV)])
        acc = _row_to_col(ws[0]) * o_all[0, u].astype(F32)
        for c in range(1, N_DEV):
            acc = acc + _row_to_col(ws[c]) * o_all[c, u].astype(F32)
        ctx_all[u] = acc.astype(BF16)

    def scores(u, qb, slot):
        k = kbuf[u].reshape(KEYS, DH).astype(BF16)
        s = lax.dot_general(q_all[slot, qb], k, (((1,), (1,)), ((), ())),
                            preferred_element_type=F32)
        m = jnp.max(s, axis=1, keepdims=True)
        p = jnp.exp2(s - m)
        l = jnp.sum(p, axis=1, keepdims=True)
        lse_all[me, u] = _col_to_row(m + jnp.log2(l))
        return p.astype(BF16), 1.0 / l

    def unit_step(u, carry):
        nxt = u + WINDOW

        @pl.when(nxt < SWAP0)
        def _():
            kv_copy(0, nxt).start()
            kv_copy(1, nxt).start()

        @pl.when(jnp.logical_and(nxt >= SWAP0, nxt < LAST))
        def _():
            kv_copy(0, nxt, 1).start()
            kv_copy(1, nxt, 1).start()

        @pl.when(nxt == LAST)
        def _():
            kv_copy(0, LAST).start()
            for j in range(len(V_CUTS) - 1):
                v_last_copy(j).start()

        @pl.when(nxt == LAST + GRP)
        def _():
            for i in range(len(PIECES)):
                late_wo_copy(i).start()

        for which in range(2):
            @pl.when(jnp.logical_and(u < LOOP_SWAPS, lax.rem(u, 2) == which))
            def _():
                target = SWAP0 + len(PRE_SWAPS) + u // 2
                swap_copy(which, target, 1 + 2 * lax.rem(target, 2)).start()

        for part, at in enumerate((0, GRP, N_EARLY)):
            @pl.when(u == at)
            def _():
                wait_bytes(q_slice(part, 1 - c_half), q_recv.at[part])

        @pl.when(u == LATE_Q_AT)
        def _():
            finish_q(2)

        wait_bytes(kbuf.at[u], ksem.at[u])
        wait_bytes(vbuf.at[u], vsem.at[u])
        p, inv_l = scores(u, *unit_coords(u))
        v = vbuf[u].reshape(KEYS, DH).astype(BF16)
        o_all[me, u] = (jnp.dot(p, v, preferred_element_type=F32) * inv_l).astype(BF16)

        unit_owner = lax.rem(u, GRP)

        @pl.when(jnp.logical_and(u < N_RS * GRP, unit_owner != me))
        def _():
            d = lax.rem(unit_owner - me + N_DEV, N_DEV)
            send_lse(u, u // GRP, d)
            send_o(u, u // GRP, d)

        @pl.when(u >= N_RS * GRP)
        def _():
            for d in tail_order:
                send_lse(u, all_slot(u), d)
                send_o(u, all_slot(u), d)

        gm = _lookup(u, MERGE_ITERS)

        @pl.when(gm >= 0)
        def _():
            mine = gm * GRP + me
            wait_lse(mine, gm)
            wait_o(mine, gm)
            merge(mine)
            for d in (1, 3, 2):
                @pl.when(jnp.logical_or(gm >= N_QB, peer(d) != IDLE_CHIP))
                def _():
                    remote(ctx_all.at[mine], c_send, c_recv.at[sem_index(gm, d)], d).start()

        gp = _lookup(u, PROJ_ITERS)

        @pl.when(jnp.logical_and(gp >= 0, owner))
        def _():
            wait_ctx(gp)

            def project_early(w):
                ctx = jnp.concatenate([ctx_all[gp * GRP + i] for i in range(GRP)], axis=1)
                osl[me, gp, :, :w] = jnp.dot(
                    ctx, wobf[:, :w], preferred_element_type=F32).astype(BF16)
                part = osl.at[me, gp, :, pl.ds(0, w)]
                remote(part, s_send, sx_recv.at[gp], d_x).start()
                remote(part, s_send, s_recv.at[0], d_q).start()

            by_width(me, project_early)

        gf = _lookup(u, FWD_ITERS)

        @pl.when(gf >= 0)
        def _():
            def forward(w):
                part = osl.at[peer(d_x), gf, :, pl.ds(0, w)]
                wait_bytes(part, sx_recv.at[gf])
                remote(part, f_send, s_recv.at[1], d_q).start()

            by_width(peer(d_x), forward)

        @pl.when(u == FOLD_AT)
        def _():
            for i, d in enumerate((d_q, 2)):
                by_width(peer(d), lambda w: wait_bytes(
                    osl.at[peer(d), :, :, pl.ds(0, w)], s_recv.at[i]))
            for chip, c0, w in OWNER_COLS:
                out_ref[0, :, c0:c0 + w] = osl[chip, :, :, :w].reshape(SQ, w).astype(F32)

        return carry

    lax.fori_loop(0, LAST, unit_step, 0)

    wait_bytes(kbuf.at[LAST], ksem.at[LAST])
    p, inv_l = scores(LAST, N_QB - 1, HQ - 1)
    for d in tail_order:
        send_lse(LAST, all_slot(LAST), d)
    acc = None
    for j in range(len(V_CUTS) - 1):
        v_last_copy(j).wait()
        b0, b1 = V_CUTS[j], V_CUTS[j + 1]
        v = vbuf[LAST, b0:b1].reshape((b1 - b0) * BLK, DH).astype(BF16)
        t = jnp.dot(p[:, b0 * BLK:b1 * BLK], v, preferred_element_type=F32)
        acc = t if acc is None else acc + t
    o_all[me, LAST] = (acc * inv_l).astype(BF16)
    for d in tail_order:
        send_o(LAST, all_slot(LAST), d)

    for g in range(N_QB, N_RS):
        wait_ctx(g)
    wait_bytes(xh.at[0], x_send)
    wait_bytes(qsend, p_send)
    wait_bytes(qsend, q_send)
    wait_bytes(kbuf.at[pl.ds(0, N_SWAPPED), pl.ds(0, 2)], w_send)

    @pl.when(owner)
    def _():
        wait_bytes(ctx_all.at[pl.ds(0, 3 * N_RS - N_QB)], c_send)

    @pl.when(jnp.logical_not(owner))
    def _():
        wait_bytes(ctx_all.at[pl.ds(0, 3 * N_RS)], c_send)

    by_width(me, lambda w: wait_bytes(osl.at[pl.ds(0, 2), :, :, pl.ds(0, w)], s_send))
    by_width(peer(d_x), lambda w: wait_bytes(osl.at[0, :, :, pl.ds(0, w)], f_send))

    head = (N_QB - 1) * BLK
    for i, (j, c0) in enumerate(PIECES):
        units = MERGE_AT.get(i, ())
        for u in units:
            wait_lse(u, all_slot(u))
            wait_o(u, all_slot(u))
        if i == WEIGHTS_AT:
            wait_lse(LAST, all_slot(LAST))
            wait_bytes(o_all.at[pl.ds(0, 3), pl.ds(0, N_SLOTS)], o_send)
            wait_bytes(lse_all.at[pl.ds(0, 3), pl.ds(0, N_SLOTS)], l_send)
        late_wo_copy(i).wait()

        wo = wolbuf[j, :, c0:c0 + HALF].astype(BF16)
        rows = SQ
        if j == GRP - 1:
            wo7bf[:, c0:c0 + HALF] = wo
            rows = head
        ctx = ctx_all[pl.ds((GRP + j) * GRP, rows // BLK)].reshape(rows, DH)
        out_ref[0, :rows, c0:c0 + HALF] = out_ref[0, :rows, c0:c0 + HALF] + jnp.dot(
            ctx, wo, preferred_element_type=F32)
        for u in units:
            merge(u)
        if i == WEIGHTS_AT:
            ws = _chip_weights([lse_all[c, LAST] for c in range(N_DEV)])
            for c in range(N_DEV):
                wcol[c] = jnp.broadcast_to(_row_to_col(ws[c]), (BLK, DH))

    wait_o(LAST, all_slot(LAST))
    acc = wcol[0] * o_all[0, LAST].astype(F32)
    for c in range(1, N_DEV):
        acc = acc + wcol[c] * o_all[c, LAST].astype(F32)
    out_ref[0, head:] = out_ref[0, head:] + jnp.dot(
        acc.astype(BF16), wo7bf[...], preferred_element_type=F32)


def pallas_dist_sparse_attn_strided_kvseq_b1_sq256_skv4096_hq8_dh128_kernel(
    x: jax.Array,
    Wq: jax.Array,
    K_ext: jax.Array,
    V_ext: jax.Array,
    Wo: jax.Array,
):
    dma = pltpu.SemaphoreType.DMA
    return pl.pallas_call(
        _body,
        out_shape=jax.ShapeDtypeStruct((1, SQ, D_MODEL), F32),
        in_specs=[pl.BlockSpec(memory_space=pl.ANY)] * 5,
        out_specs=pl.BlockSpec(memory_space=pltpu.VMEM),
        scratch_shapes=[
            pltpu.VMEM((N_UNITS, N_KB, BLK, DH), F32),
            pltpu.VMEM((N_UNITS, N_KB, BLK, DH), F32),
            pltpu.VMEM((SQ // 2, HALF), F32),
            pltpu.VMEM((2, SQ // 2, HALF), BF16),
            pltpu.VMEM((HALF, HALF), F32),
            pltpu.VMEM((HALF, HALF), BF16),
            pltpu.VMEM((GRP, N_QB, BLK, DH), F32),
            pltpu.VMEM((GRP, N_QB, BLK, DH), BF16),
            pltpu.VMEM((GRP, N_QB, BLK, DH), BF16),
            pltpu.VMEM((2, 2 * DH, WIDE), F32),
            pltpu.VMEM((GRP * DH, WIDE), BF16),
            pltpu.VMEM((GRP, DH, D_MODEL), F32),
            pltpu.VMEM((DH, D_MODEL), BF16),
            pltpu.VMEM((HQ, N_QB, BLK, DH), BF16),
            pltpu.VMEM((N_DEV, N_UNITS, BLK, DH), BF16),
            pltpu.VMEM((N_DEV, N_UNITS, 1, DH), F32),
            pltpu.VMEM((N_UNITS, BLK, DH), BF16),
            pltpu.VMEM((N_DEV, N_QB, BLK, WIDE), BF16),
            pltpu.VMEM((N_DEV, BLK, DH), F32),
            dma((N_UNITS,)),
            dma((LAST,)),
            dma((len(V_CUTS) - 1,)),
            dma((3,)),
            dma((len(PIECES),)),
            dma((9,)),
            dma,
            dma((len(Q_PARTS),)),
            dma((len(Q_PARTS),)),
            dma((3 * N_SLOTS,)),
            dma((3 * N_SLOTS,)),
            dma((3 * N_RS,)),
            dma((N_QB,)),
            dma((2,)),
        ],
        compiler_params=pltpu.CompilerParams(
            collective_id=0,
            vmem_limit_bytes=64 * 1024 * 1024,
            disable_semaphore_checks=True,
        ),
    )(x, Wq,
      K_ext.reshape(N_KB, N_QB, BLK, HQ, DH),
      V_ext.reshape(N_KB, N_QB, BLK, HQ, DH),
      Wo.reshape(2, 2, 2 * DH, D_MODEL))
```

```python
import jax
import jax.numpy as jnp
from jax import lax
from jax.experimental import pallas as pl
from jax.experimental.pallas import tpu as pltpu

N_DEV = 4
SQ = 256
D_MODEL = 1024
HALF = D_MODEL // 2
HQ = 8
DH = 128
BLK = 64
N_QB = SQ // BLK
N_KB = 16
KEYS = N_KB * BLK
GRP = 4
N_EARLY = N_QB * GRP
N_UNITS = N_QB * HQ
LAST = N_UNITS - 1
N_RS = 6
N_SLOTS = N_RS + N_UNITS - N_RS * GRP
WINDOW = 10

MERGE_ITERS = (9, 11, 14, 18, 22, 26)
PROJ_ITERS = (12, 15, 18, 21)
FWD_ITERS = (15, 18, 21, 24)
LATE_Q_AT = 3
FOLD_AT = 29

WIDE = 384
NARROW = 256
IDLE_CHIP = 2
NARROW_CHIP = 1
OWNER_COLS = ((0, 0, WIDE), (1, WIDE, NARROW), (3, WIDE + NARROW, WIDE))

PRE_SWAPS = ((1, "q", 0, 0), (2, "q", 0, 1), (3, "q", 1, 1),
             (4, "x", 2, 2), (6, "x", 3, 3), (8, "x", 4, 4))
LEAD = 5
SIDE_ITERS = 28
RING = 4
N_SWAPPED = len(PRE_SWAPS) + SIDE_ITERS // 4

V_CUTS = (0, 12, 16)
PIECES = tuple((j, c) for j in range(GRP) for c in (0, HALF))
MERGE_AT = {0: (24, 25), 1: (26, 27), 2: (28,), 3: (29,), 5: (30,)}
WEIGHTS_AT = 6
Q_PARTS = ((0, 0, 1), (0, 1, N_QB - 1), (1, 0, N_QB))

SCALE_LOG2 = 0.08838834764831843 * 1.4426950408889634
MESH = pl.DeviceIdType.MESH
F32 = jnp.float32
BF16 = jnp.bfloat16


def _diagonal(val):
    r = lax.broadcasted_iota(jnp.int32, (BLK, DH), 0)
    c = lax.broadcasted_iota(jnp.int32, (BLK, DH), 1)
    return jnp.where(r == c, val, 0.0)


def _col_to_row(col):
    return jnp.sum(_diagonal(col), axis=0, keepdims=True)


def _row_to_col(row):
    return jnp.sum(_diagonal(row), axis=1, keepdims=True)


def _chip_weights(lses):
    m = jnp.maximum(jnp.maximum(lses[0], lses[1]), jnp.maximum(lses[2], lses[3]))
    es = [jnp.exp2(t - m) for t in lses]
    inv = 1.0 / (es[0] + es[1] + es[2] + es[3])
    return [e * inv for e in es]


def _lookup(u, iters):
    r = jnp.int32(-1)
    for g, at in enumerate(iters):
        r = jnp.where(u == at, g, r)
    return r


def _body(x_hbm, wq_hbm, k_hbm, v_hbm, wo_hbm, out_ref,
          kbuf, vbuf, xbuf, xh, wqbuf, wqbf, qpart, qsend, qrecv, wobuf, wobf, wolbuf,
          wo7bf, q_all, o_all, lse_all, ctx_all, osl, wcol, stage,
          ksem, vsem, vlsem, insem, wolsem, stsem,
          send, x_recv, p_recv, q_recv, o_recv, l_recv, c_recv, sx_recv, s_recv):
    me = lax.axis_index("i")
    odd = lax.rem(me, 2) == 1
    owner = me != IDLE_CHIP
    k_half = me // 2
    c_half = lax.rem((me + 1) // 2, 2)
    d_x = jnp.where(odd, 3, 1)
    d_q = jnp.where(odd, 1, 3)
    first = jnp.where(odd, N_DEV - me, 2)
    second = jnp.where(odd, 2, 1)
    tail_order = (first, second, 6 - first - second)
    (x_send, p_send, q_send, o_send, l_send, c_send, s_send, f_send, w_send) = (
        send.at[i] for i in range(9))
    kv = ((k_hbm, kbuf, ksem), (v_hbm, vbuf, vsem))

    def peer(d):
        return lax.rem(me + d, N_DEV)

    def source(d):
        return lax.rem(me + (N_DEV - d), N_DEV)

    def unit_coords(u):
        hi, lo = u // GRP, lax.rem(u, GRP)
        early = u < N_EARLY
        return jnp.where(early, hi, lo), jnp.where(early, lo, hi)

    def unit_src(src, u, blocks):
        qb, slot = unit_coords(u)
        idx = lax.rem(slot, GRP)
        head = (idx // 2) * GRP + (slot // GRP) * 2 + lax.rem(idx, 2)
        return src.at[blocks, qb, :, head, :]

    def kv_copy(which, u, first_block=0):
        src, dst, sem = kv[which]
        blocks = pl.ds(first_block, N_KB - first_block)
        return pltpu.make_async_copy(unit_src(src, u, blocks), dst.at[u, blocks], sem.at[u])

    def swap_copy(which, u, d):
        src, dst, sem = kv[which]
        block = pl.ds(0, 1)
        return pltpu.make_async_remote_copy(
            src_ref=unit_src(src, u, block), dst_ref=dst.at[u, block],
            send_sem=w_send, recv_sem=sem.at[u],
            device_id=(peer(d),), device_id_type=MESH)

    def pre_swaps(point):
        for u, link, *points in PRE_SWAPS:
            for which in range(2):
                if points[which] == point:
                    swap_copy(which, u, d_q if link == "q" else d_x).start()

    def fetch(which, u, slot, block=0):
        pltpu.make_async_copy(
            unit_src(kv[which][0], u, block), stage.at[slot], stsem.at[slot]).start()

    def deliver(which, u, slot, block=0):
        _, dst, sem = kv[which]
        wait_bytes(stage.at[slot], stsem.at[slot])
        pltpu.make_async_copy(stage.at[slot], dst.at[u, block], sem.at[u]).start()

    def v_last_sem(j):
        return vsem.at[LAST] if j == len(V_CUTS) - 2 else vlsem.at[j]

    def v_last_copy(j):
        blocks = pl.ds(V_CUTS[j], min(V_CUTS[j + 1], N_KB - 1) - V_CUTS[j])
        return pltpu.make_async_copy(
            unit_src(v_hbm, LAST, blocks), vbuf.at[LAST, blocks], v_last_sem(j))

    def late_wo_copy(i):
        j, c0 = PIECES[i]
        return pltpu.make_async_copy(
            wo_hbm.at[j // 2, 1, pl.ds((j % 2) * DH, DH), pl.ds(c0, HALF)],
            wolbuf.at[j, :, pl.ds(c0, HALF)], wolsem.at[i])

    def early_wo_copy(w):
        col0 = jnp.int32(0)
        for chip, start, _ in OWNER_COLS:
            col0 = jnp.where(me == chip, start, col0)
        return pltpu.make_async_copy(
            wo_hbm.at[:, 0, :, pl.ds(pl.multiple_of(col0, DH), w)],
            wobuf.at[:, :, pl.ds(0, w)], insem.at[2])

    def remote(ref, send_sem, recv_sem, d):
        return pltpu.make_async_remote_copy(
            src_ref=ref, dst_ref=ref, send_sem=send_sem, recv_sem=recv_sem,
            device_id=(peer(d),), device_id_type=MESH)

    def wait_bytes(ref, sem):
        pltpu.make_async_copy(ref, ref, sem).wait()

    def by_width(chip, fn):
        @pl.when(jnp.logical_and(chip != IDLE_CHIP, chip != NARROW_CHIP))
        def _():
            fn(WIDE)

        @pl.when(chip == NARROW_CHIP)
        def _():
            fn(NARROW)

    k_rows = pl.ds(pl.multiple_of(k_half * HALF, HALF), HALF)
    x_copy = pltpu.make_async_copy(
        x_hbm.at[0, pl.ds(pl.multiple_of(c_half * (SQ // 2), SQ // 2), SQ // 2), k_rows],
        xbuf, insem.at[0])
    wq_copy = pltpu.make_async_copy(
        wq_hbm.at[k_rows, pl.ds(pl.multiple_of(c_half * HALF, HALF), HALF)],
        wqbuf, insem.at[1])

    x_copy.start()
    barrier = pltpu.get_barrier_semaphore()
    for d in (2, 1, 3):
        pl.semaphore_signal(barrier, inc=1, device_id=(peer(d),), device_id_type=MESH)
    wq_copy.start()
    by_width(me, lambda w: early_wo_copy(w).start())
    for which in range(2):
        fetch(which, 0, RING + which)
    for u in range(WINDOW):
        kv_copy(0, u, 1).start()
        kv_copy(1, u, 1).start()

    x_copy.wait()
    xh[c_half] = xbuf[...].astype(BF16)
    pl.semaphore_wait(barrier, N_DEV - 1)
    remote(xh.at[c_half], x_send, x_recv, d_x).start()
    pre_swaps(0)
    wq_copy.wait()
    wqbf[...] = wqbuf[...].astype(BF16)

    def load_early_wo(w):
        early_wo_copy(w).wait()
        wobf[:, :w] = wobuf[:, :, :w].reshape(GRP * DH, w).astype(BF16)

    by_width(me, load_early_wo)
    for which in range(2):
        deliver(which, 0, RING + which)
    pre_swaps(1)
    wait_bytes(xh.at[1 - c_half], x_recv)
    pre_swaps(2)
    q = jnp.dot(xh[...].reshape(SQ, HALF), wqbf[...],
                preferred_element_type=F32) * SCALE_LOG2
    for j in range(GRP):
        qj = q[:, j * DH:(j + 1) * DH].reshape(N_QB, BLK, DH)
        qpart[j] = qj
        qsend[j] = qj.astype(BF16)

    def p_slice(ref, part):
        late, q0, nq = Q_PARTS[part]
        return ref.at[pl.ds(2 * late, 2), pl.ds(q0, nq)]

    def q_slice(part, half):
        late, q0, nq = Q_PARTS[part]
        return q_all.at[pl.ds(late * GRP + 2 * half, 2), pl.ds(q0, nq)]

    for part in range(len(Q_PARTS)):
        pltpu.make_async_remote_copy(
            src_ref=p_slice(qsend, part), dst_ref=p_slice(qrecv, part), send_sem=p_send,
            recv_sem=p_recv.at[part], device_id=(peer(d_q),), device_id_type=MESH).start()

    def finish_q(part):
        wait_bytes(p_slice(qrecv, part), p_recv.at[part])
        q_slice(part, c_half)[...] = (
            p_slice(qpart, part)[...] + p_slice(qrecv, part)[...].astype(F32)).astype(BF16)
        remote(q_slice(part, c_half), q_send, q_recv.at[part], d_x).start()

    pre_swaps(3)
    finish_q(0)
    pre_swaps(4)
    finish_q(1)

    def sem_index(slot, d):
        return slot * 3 + d - 1

    def all_slot(u):
        return u - N_RS * (GRP - 1)

    def send_lse(u, slot, d):
        remote(lse_all.at[me, u], l_send, l_recv.at[sem_index(slot, d)], d).start()

    def send_o(u, slot, d):
        remote(o_all.at[me, u], o_send, o_recv.at[sem_index(slot, d)], d).start()

    def wait_lse(u, slot):
        for d in (1, 2, 3):
            wait_bytes(lse_all.at[source(d), u], l_recv.at[sem_index(slot, d)])

    def wait_o(u, slot):
        for d in (1, 2, 3):
            wait_bytes(o_all.at[source(d), u], o_recv.at[sem_index(slot, d)])

    def wait_ctx(g):
        for d in (1, 2, 3):
            wait_bytes(ctx_all.at[g * GRP + source(d)], c_recv.at[sem_index(g, d)])

    def merge(u):
        ws = _chip_weights([lse_all[c, u] for c in range(N_DEV)])
        acc = _row_to_col(ws[0]) * o_all[0, u].astype(F32)
        for c in range(1, N_DEV):
            acc = acc + _row_to_col(ws[c]) * o_all[c, u].astype(F32)
        ctx_all[u] = acc.astype(BF16)

    def scores(u, qb, slot):
        k = kbuf[u].reshape(KEYS, DH).astype(BF16)
        s = lax.dot_general(q_all[slot, qb], k, (((1,), (1,)), ((), ())),
                            preferred_element_type=F32)
        m = jnp.max(s, axis=1, keepdims=True)
        p = jnp.exp2(s - m)
        l = jnp.sum(p, axis=1, keepdims=True)
        lse_all[me, u] = _col_to_row(m + jnp.log2(l))
        return p.astype(BF16), 1.0 / l

    def unit_step(u, carry):
        nxt = u + WINDOW

        side = jnp.logical_or(lax.rem(nxt, 2) == 1, nxt == LAST - 1)

        @pl.when(jnp.logical_and(nxt < LAST, jnp.logical_not(side)))
        def _():
            kv_copy(0, nxt).start()
            kv_copy(1, nxt).start()

        @pl.when(jnp.logical_and(nxt < LAST, side))
        def _():
            kv_copy(0, nxt, 1).start()
            kv_copy(1, nxt, 1).start()

        @pl.when(nxt == LAST)
        def _():
            kv_copy(0, LAST, 1).start()
            for j in range(len(V_CUTS) - 1):
                v_last_copy(j).start()

        @pl.when(nxt == LAST + GRP)
        def _():
            for i in range(len(PIECES)):
                late_wo_copy(i).start()

        for which in range(2):
            target = u + LEAD - which
            turn = lax.rem(u // 4, 2)

            @pl.when(jnp.logical_and(u < SIDE_ITERS, lax.rem(u, 4) == which))
            def _():
                fetch(which, target, 2 * turn + which)

            @pl.when(jnp.logical_and(u < SIDE_ITERS, lax.rem(u, 4) == 2 + which))
            def _():
                deliver(which, target - 2, 2 * turn + which)
                swap_copy(which, jnp.minimum(target, LAST - 1), 1 + 2 * turn).start()

        for which, block in enumerate((0, N_KB - 1)):
            @pl.when(u == SIDE_ITERS + which + 1)
            def _():
                deliver(which, LAST, RING + which, block)

        for which, block in enumerate((0, N_KB - 1)):
            @pl.when(u == SIDE_ITERS + which)
            def _():
                fetch(which, LAST, RING + which, block)

        for part, at in enumerate((0, GRP, N_EARLY)):
            @pl.when(u == at)
            def _():
                wait_bytes(q_slice(part, 1 - c_half), q_recv.at[part])

        @pl.when(u == LATE_Q_AT)
        def _():
            finish_q(2)

        wait_bytes(kbuf.at[u], ksem.at[u])
        wait_bytes(vbuf.at[u], vsem.at[u])
        p, inv_l = scores(u, *unit_coords(u))
        v = vbuf[u].reshape(KEYS, DH).astype(BF16)
        o_all[me, u] = (jnp.dot(p, v, preferred_element_type=F32) * inv_l).astype(BF16)

        unit_owner = lax.rem(u, GRP)

        @pl.when(jnp.logical_and(u < N_RS * GRP, unit_owner != me))
        def _():
            d = lax.rem(unit_owner - me + N_DEV, N_DEV)
            send_lse(u, u // GRP, d)
            send_o(u, u // GRP, d)

        @pl.when(u >= N_RS * GRP)
        def _():
            for d in tail_order:
                send_lse(u, all_slot(u), d)
                send_o(u, all_slot(u), d)

        gm = _lookup(u, MERGE_ITERS)

        @pl.when(gm >= 0)
        def _():
            mine = gm * GRP + me
            wait_lse(mine, gm)
            wait_o(mine, gm)
            merge(mine)
            for d in (1, 3, 2):
                @pl.when(jnp.logical_or(gm >= N_QB, peer(d) != IDLE_CHIP))
                def _():
                    remote(ctx_all.at[mine], c_send, c_recv.at[sem_index(gm, d)], d).start()

        gp = _lookup(u, PROJ_ITERS)

        @pl.when(jnp.logical_and(gp >= 0, owner))
        def _():
            wait_ctx(gp)

            def project_early(w):
                ctx = jnp.concatenate([ctx_all[gp * GRP + i] for i in range(GRP)], axis=1)
                osl[me, gp, :, :w] = jnp.dot(
                    ctx, wobf[:, :w], preferred_element_type=F32).astype(BF16)
                part = osl.at[me, gp, :, pl.ds(0, w)]
                remote(part, s_send, sx_recv.at[gp], d_x).start()
                remote(part, s_send, s_recv.at[0], d_q).start()

            by_width(me, project_early)

        gf = _lookup(u, FWD_ITERS)

        @pl.when(gf >= 0)
        def _():
            def forward(w):
                part = osl.at[peer(d_x), gf, :, pl.ds(0, w)]
                wait_bytes(part, sx_recv.at[gf])
                remote(part, f_send, s_recv.at[1], d_q).start()

            by_width(peer(d_x), forward)

        @pl.when(u == FOLD_AT)
        def _():
            for i, d in enumerate((d_q, 2)):
                by_width(peer(d), lambda w: wait_bytes(
                    osl.at[peer(d), :, :, pl.ds(0, w)], s_recv.at[i]))
            for chip, c0, w in OWNER_COLS:
                out_ref[0, :, c0:c0 + w] = osl[chip, :, :, :w].reshape(SQ, w).astype(F32)

        return carry

    lax.fori_loop(0, LAST, unit_step, 0)

    wait_bytes(kbuf.at[LAST], ksem.at[LAST])
    p, inv_l = scores(LAST, N_QB - 1, HQ - 1)
    for d in tail_order:
        send_lse(LAST, all_slot(LAST), d)
    acc = None
    for j in range(len(V_CUTS) - 1):
        b0, b1 = V_CUTS[j], V_CUTS[j + 1]
        wait_bytes(vbuf.at[LAST, pl.ds(b0, b1 - b0)], v_last_sem(j))
        v = vbuf[LAST, b0:b1].reshape((b1 - b0) * BLK, DH).astype(BF16)
        t = jnp.dot(p[:, b0 * BLK:b1 * BLK], v, preferred_element_type=F32)
        acc = t if acc is None else acc + t
    o_all[me, LAST] = (acc * inv_l).astype(BF16)
    for d in tail_order:
        send_o(LAST, all_slot(LAST), d)

    for g in range(N_QB, N_RS):
        wait_ctx(g)
    wait_bytes(xh.at[0], x_send)
    wait_bytes(qsend, p_send)
    wait_bytes(qsend, q_send)
    wait_bytes(kbuf.at[pl.ds(0, N_SWAPPED), pl.ds(0, 2)], w_send)

    @pl.when(owner)
    def _():
        wait_bytes(ctx_all.at[pl.ds(0, 3 * N_RS - N_QB)], c_send)

    @pl.when(jnp.logical_not(owner))
    def _():
        wait_bytes(ctx_all.at[pl.ds(0, 3 * N_RS)], c_send)

    by_width(me, lambda w: wait_bytes(osl.at[pl.ds(0, 2), :, :, pl.ds(0, w)], s_send))
    by_width(peer(d_x), lambda w: wait_bytes(osl.at[0, :, :, pl.ds(0, w)], f_send))

    head = (N_QB - 1) * BLK
    for i, (j, c0) in enumerate(PIECES):
        units = MERGE_AT.get(i, ())
        for u in units:
            wait_lse(u, all_slot(u))
            wait_o(u, all_slot(u))
        if i == WEIGHTS_AT:
            wait_lse(LAST, all_slot(LAST))
            wait_bytes(o_all.at[pl.ds(0, 3), pl.ds(0, N_SLOTS)], o_send)
            wait_bytes(lse_all.at[pl.ds(0, 3), pl.ds(0, N_SLOTS)], l_send)
        late_wo_copy(i).wait()

        wo = wolbuf[j, :, c0:c0 + HALF].astype(BF16)
        rows = SQ
        if j == GRP - 1:
            wo7bf[:, c0:c0 + HALF] = wo
            rows = head
        ctx = ctx_all[pl.ds((GRP + j) * GRP, rows // BLK)].reshape(rows, DH)
        out_ref[0, :rows, c0:c0 + HALF] = out_ref[0, :rows, c0:c0 + HALF] + jnp.dot(
            ctx, wo, preferred_element_type=F32)
        for u in units:
            merge(u)
        if i == WEIGHTS_AT:
            ws = _chip_weights([lse_all[c, LAST] for c in range(N_DEV)])
            for c in range(N_DEV):
                wcol[c] = jnp.broadcast_to(_row_to_col(ws[c]), (BLK, DH))

    wait_o(LAST, all_slot(LAST))
    acc = wcol[0] * o_all[0, LAST].astype(F32)
    for c in range(1, N_DEV):
        acc = acc + wcol[c] * o_all[c, LAST].astype(F32)
    out_ref[0, head:] = out_ref[0, head:] + jnp.dot(
        acc.astype(BF16), wo7bf[...], preferred_element_type=F32)


def pallas_dist_sparse_attn_strided_kvseq_b1_sq256_skv4096_hq8_dh128_kernel(
    x: jax.Array,
    Wq: jax.Array,
    K_ext: jax.Array,
    V_ext: jax.Array,
    Wo: jax.Array,
):
    dma = pltpu.SemaphoreType.DMA
    return pl.pallas_call(
        _body,
        out_shape=jax.ShapeDtypeStruct((1, SQ, D_MODEL), F32),
        in_specs=[pl.BlockSpec(memory_space=pl.ANY)] * 5,
        out_specs=pl.BlockSpec(memory_space=pltpu.VMEM),
        scratch_shapes=[
            pltpu.VMEM((N_UNITS, N_KB, BLK, DH), F32),
            pltpu.VMEM((N_UNITS, N_KB, BLK, DH), F32),
            pltpu.VMEM((SQ // 2, HALF), F32),
            pltpu.VMEM((2, SQ // 2, HALF), BF16),
            pltpu.VMEM((HALF, HALF), F32),
            pltpu.VMEM((HALF, HALF), BF16),
            pltpu.VMEM((GRP, N_QB, BLK, DH), F32),
            pltpu.VMEM((GRP, N_QB, BLK, DH), BF16),
            pltpu.VMEM((GRP, N_QB, BLK, DH), BF16),
            pltpu.VMEM((2, 2 * DH, WIDE), F32),
            pltpu.VMEM((GRP * DH, WIDE), BF16),
            pltpu.VMEM((GRP, DH, D_MODEL), F32),
            pltpu.VMEM((DH, D_MODEL), BF16),
            pltpu.VMEM((HQ, N_QB, BLK, DH), BF16),
            pltpu.VMEM((N_DEV, N_UNITS, BLK, DH), BF16),
            pltpu.VMEM((N_DEV, N_UNITS, 1, DH), F32),
            pltpu.VMEM((N_UNITS, BLK, DH), BF16),
            pltpu.VMEM((N_DEV, N_QB, BLK, WIDE), BF16),
            pltpu.VMEM((N_DEV, BLK, DH), F32),
            pltpu.SMEM((RING + 2, BLK, DH), F32),
            dma((N_UNITS,)),
            dma((N_UNITS,)),
            dma((len(V_CUTS) - 2,)),
            dma((3,)),
            dma((len(PIECES),)),
            dma((RING + 2,)),
            dma((9,)),
            dma,
            dma((len(Q_PARTS),)),
            dma((len(Q_PARTS),)),
            dma((3 * N_SLOTS,)),
            dma((3 * N_SLOTS,)),
            dma((3 * N_RS,)),
            dma((N_QB,)),
            dma((2,)),
        ],
        compiler_params=pltpu.CompilerParams(
            collective_id=0,
            vmem_limit_bytes=64 * 1024 * 1024,
            disable_semaphore_checks=True,
        ),
    )(x, Wq,
      K_ext.reshape(N_KB, N_QB, BLK, HQ, DH),
      V_ext.reshape(N_KB, N_QB, BLK, HQ, DH),
      Wo.reshape(2, 2, 2 * DH, D_MODEL))
```
